```python
import numpy as np

kernel_name = "dist_rope_attn_htp_bs_b2_sq512_d1024_hq8_dh128"

def setup_inputs():
    x = np.random.randn(8, 512, 1024).astype(np.float32)
    Wq = np.random.randn(1024, 4096).astype(np.float32) * 0.02
    Wk = np.random.randn(1024, 4096).astype(np.float32) * 0.02
    Wv = np.random.randn(1024, 4096).astype(np.float32) * 0.02
    Wo = np.random.randn(4096, 1024).astype(np.float32) * 0.02
    return {"x": x, "Wq": Wq, "Wk": Wk, "Wv": Wv, "Wo": Wo}

def reference(x, Wq, Wk, Wv, Wo):
    B, Sq, Hq, Dh = 8, 512, 32, 128
    inv = 1.0 / (10000.0 ** (np.arange(0, Dh, 2) / Dh))
    pos = np.arange(Sq)[:, None] * inv[None, :]
    cos = np.repeat(np.cos(pos), 2, axis=-1).astype(np.float32)
    sin = np.repeat(np.sin(pos), 2, axis=-1).astype(np.float32)
    def rot(t):
        t2 = t.reshape(B, Sq, Hq, Dh // 2, 2)
        t_r = np.stack([-t2[..., 1], t2[..., 0]], axis=-1).reshape(B, Sq, Hq, Dh)
        return t * cos[None, :, None, :] + t_r * sin[None, :, None, :]
    Q = rot((x @ Wq).reshape(B, Sq, Hq, Dh))
    K = rot((x @ Wk).reshape(B, Sq, Hq, Dh))
    V = (x @ Wv).reshape(B, Sq, Hq, Dh)
    s = np.einsum('bihd,bjhd->bhij', Q, K).astype(np.float32) * 0.08838834764831843
    s_max = s.max(axis=-1, keepdims=True)
    w = np.exp(s - s_max)
    w = w / w.sum(axis=-1, keepdims=True)
    ctx = np.einsum('bhij,bjhd->bihd', w, V).reshape(B, Sq, Hq * Dh)
    return ctx @ Wo
```

```python
import numpy as np

import jax
import jax.numpy as jnp
from jax import lax
from jax.experimental import pallas as pl
from jax.experimental.pallas import tpu as pltpu

N_DEV = 4
B_LOC = 2
SQ = 512
D = 1024
H_LOC = 8
DH = 128
HD = H_LOC * DH
SCALE = 0.08838834764831843
LOG2E = 1.4426950408889634

BF16 = jnp.bfloat16
F32 = jnp.float32


def _rope_tables():
    inv = 1.0 / (10000.0 ** (np.arange(0, DH, 2) / DH))
    pos = np.arange(SQ)[:, None] * inv[None, :]
    cos = np.repeat(np.cos(pos), 2, axis=-1).astype(np.float32)
    sin = np.repeat(np.sin(pos), 2, axis=-1).astype(np.float32)
    sign = np.where(np.arange(DH) % 2 == 0, -1.0, 1.0).astype(np.float32)
    return np.stack([cos, sin * sign[None, :]]).astype(np.float32)


_TABLES = _rope_tables()


def pallas_dist_rope_attn_htp_bs_b2_sq512_d1024_hq8_dh128_kernel(
    x: jax.Array,
    Wq: jax.Array,
    Wk: jax.Array,
    Wv: jax.Array,
    Wo: jax.Array,
):
    def body(x_hbm, wq_hbm, wk_hbm, wv_hbm, wo_hbm, tab_ref, out_hbm,
             xs, wqkv, wo, wstage, xstage, tabs, q_s, k_s, v_s, ctx_s,
             res, snd, rcv, ostage,
             ld_sems, ag_send, ag_recv, rs_send, rs_recv, out_sems):
        me = lax.axis_index("i")
        left = lax.rem(me + N_DEV - 1, N_DEV)
        right = lax.rem(me + 1, N_DEV)

        def rdma(src, dst, ssem, rsem, dev):
            return pltpu.make_async_remote_copy(
                src_ref=src, dst_ref=dst, send_sem=ssem, recv_sem=rsem,
                device_id=(dev,), device_id_type=pl.DeviceIdType.MESH)

        ag = [
            rdma(xs.at[0], xs.at[2], ag_send.at[0], ag_recv.at[2], right),
            rdma(xs.at[7], xs.at[1], ag_send.at[1], ag_recv.at[1], left),
            rdma(xs.at[2], xs.at[3], ag_send.at[2], ag_recv.at[3], right),
            rdma(xs.at[1], xs.at[4], ag_send.at[3], ag_recv.at[4], left),
            rdma(xs.at[7], xs.at[6], ag_send.at[4], ag_recv.at[6], right),
            rdma(xs.at[0], xs.at[5], ag_send.at[5], ag_recv.at[5], left),
        ]
        ag_by_dst = {2: ag[0], 1: ag[1], 3: ag[2], 4: ag[3], 6: ag[4], 5: ag[5]}
        rs_plan = {1: (1, right), 2: (0, left), 3: (2, right), 4: (3, left),
                   5: (4, right), 6: (5, left)}
        rs = {u: rdma(snd.at[u], rcv.at[slot], rs_send.at[u], rs_recv.at[slot], dev)
              for u, (slot, dev) in rs_plan.items()}
        rs_by_slot = {slot: rs[u] for u, (slot, _) in rs_plan.items()}

        ld_x0 = pltpu.make_async_copy(x_hbm.at[0], xstage.at[0], ld_sems.at[0])
        ld_x1 = pltpu.make_async_copy(x_hbm.at[1], xstage.at[1], ld_sems.at[1])
        ld_w = [pltpu.make_async_copy(w, wstage.at[j], ld_sems.at[2 + j])
                for j, w in enumerate((wq_hbm, wk_hbm, wv_hbm, wo_hbm))]
        ld_x0.start()
        ld_x1.start()
        for c in ld_w:
            c.start()

        barrier = pltpu.get_barrier_semaphore()
        for nbr in (left, right):
            pl.semaphore_signal(barrier, inc=1, device_id=(nbr,),
                                device_id_type=pl.DeviceIdType.MESH)

        tabs[0] = tab_ref[0]
        tabs[1] = tab_ref[1]
        tabs[2] = tab_ref[0] * (SCALE * LOG2E)
        tabs[3] = tab_ref[1] * (SCALE * LOG2E)
        rcv[6] = jnp.zeros((SQ, D), BF16)

        ld_x0.wait()
        xs[0] = xstage[0].astype(BF16)
        ld_x1.wait()
        xs[7] = xstage[1].astype(BF16)
        pl.semaphore_wait(barrier, 2)
        ag[0].start()
        ag[1].start()

        for j in range(3):
            ld_w[j].wait()
            wqkv[j] = wstage[j].astype(BF16)
        ld_w[3].wait()
        wo[...] = wstage[3].astype(BF16)

        even = (lax.broadcasted_iota(jnp.int32, (SQ, DH), 1) % 2) == 0

        def rope(t, c, s):
            sw = jnp.where(even, pltpu.roll(t, DH - 1, 1), pltpu.roll(t, 1, 1))
            return t * c + sw * s

        def unit(u, carry):
            for k in (3, 4, 5, 6):
                @pl.when(u == k)
                def _():
                    ag_by_dst[k].wait_recv()
            @pl.when(u == 5)
            def _():
                rs_by_slot[2].wait_recv()
            @pl.when(u == 6)
            def _():
                rs_by_slot[3].wait_recv()
            @pl.when(u == 7)
            def _():
                rs_by_slot[1].wait_recv()

            xu = xs[u]
            G = 2 * DH
            for g in range(HD // G):
                cols = slice(g * G, (g + 1) * G)
                q = jnp.dot(xu, wqkv[0, :, cols], preferred_element_type=F32)
                k = jnp.dot(xu, wqkv[1, :, cols], preferred_element_type=F32)
                v = jnp.dot(xu, wqkv[2, :, cols], preferred_element_type=F32)
                v_s[:, cols] = v.astype(BF16)
                for hh in range(2):
                    sl = slice(hh * DH, (hh + 1) * DH)
                    oc = slice(g * G + hh * DH, g * G + (hh + 1) * DH)
                    q_s[:, oc] = rope(q[:, sl], tabs[2], tabs[3]).astype(BF16)
                    k_s[:, oc] = rope(k[:, sl], tabs[0], tabs[1]).astype(BF16)

            for h in range(H_LOC):
                oc = slice(h * DH, (h + 1) * DH)
                s = lax.dot_general(q_s[:, oc], k_s[:, oc],
                                    (((1,), (1,)), ((), ())),
                                    preferred_element_type=F32)
                m = jnp.max(s, axis=-1, keepdims=True)
                p = jnp.exp2(s - m)
                l = jnp.sum(p, axis=-1, keepdims=True)
                o = jnp.dot(p.astype(BF16), v_s[:, oc], preferred_element_type=F32)
                ctx_s[:, oc] = (o / l).astype(BF16)

            a = jnp.where(u == 5, 2, jnp.where(u == 6, 3, jnp.where(u == 7, 1, 6)))
            r = jnp.dot(ctx_s[...], wo[...], preferred_element_type=F32)
            r = r + rcv[a].astype(F32)
            res[jnp.where(u == 0, 0, 1)] = r
            snd[u] = r.astype(BF16)

            @pl.when(u == 0)
            def _():
                ag_by_dst[2].wait_recv()
                ag[2].start()
                ag_by_dst[1].wait_recv()
                ag[3].start()
                ag[4].start()
                ag[5].start()
            for k in range(1, 7):
                @pl.when(u == k)
                def _():
                    rs[k].start()
            @pl.when(u == 6)
            def _():
                rs_by_slot[0].wait_recv()
                rs_by_slot[4].wait_recv()
                ostage[0] = res[0] + rcv[0].astype(F32) + rcv[4].astype(F32)
                pltpu.make_async_copy(ostage.at[0], out_hbm.at[0], out_sems.at[0]).start()
            return carry

        lax.fori_loop(0, 8, unit, 0)

        rs_by_slot[5].wait_recv()
        ostage[1] = res[1] + rcv[5].astype(F32)
        o1 = pltpu.make_async_copy(ostage.at[1], out_hbm.at[1], out_sems.at[1])
        o1.start()
        for c in ag:
            c.wait_send()
        for u in range(1, 7):
            rs[u].wait_send()
        pltpu.make_async_copy(ostage.at[0], out_hbm.at[0], out_sems.at[0]).wait()
        o1.wait()

    hbm = pl.BlockSpec(memory_space=pl.ANY)
    return pl.pallas_call(
        body,
        out_shape=jax.ShapeDtypeStruct((B_LOC, SQ, D), F32),
        in_specs=[hbm, hbm, hbm, hbm, hbm,
                  pl.BlockSpec(memory_space=pltpu.VMEM)],
        out_specs=hbm,
        scratch_shapes=[
            pltpu.VMEM((8, SQ, D), BF16),
            pltpu.VMEM((3, D, HD), BF16),
            pltpu.VMEM((HD, D), BF16),
            pltpu.VMEM((4, D, HD), F32),
            pltpu.VMEM((2, SQ, D), F32),
            pltpu.VMEM((4, SQ, DH), F32),
            pltpu.VMEM((SQ, HD), BF16),
            pltpu.VMEM((SQ, HD), BF16),
            pltpu.VMEM((SQ, HD), BF16),
            pltpu.VMEM((SQ, HD), BF16),
            pltpu.VMEM((2, SQ, D), F32),
            pltpu.VMEM((8, SQ, D), BF16),
            pltpu.VMEM((7, SQ, D), BF16),
            pltpu.VMEM((2, SQ, D), F32),
            pltpu.SemaphoreType.DMA((6,)),
            pltpu.SemaphoreType.DMA((6,)),
            pltpu.SemaphoreType.DMA((8,)),
            pltpu.SemaphoreType.DMA((8,)),
            pltpu.SemaphoreType.DMA((6,)),
            pltpu.SemaphoreType.DMA((2,)),
        ],
        compiler_params=pltpu.CompilerParams(
            collective_id=0,
            vmem_limit_bytes=100 * 1024 * 1024,
        ),
    )(x, Wq, Wk, Wv, Wo, jnp.asarray(_TABLES))
```

```python
import numpy as np

import jax
import jax.numpy as jnp
from jax import lax
from jax.experimental import pallas as pl
from jax.experimental.pallas import tpu as pltpu

N_DEV = 4
B_LOC = 2
SQ = 512
D = 1024
H_LOC = 8
DH = 128
HD = H_LOC * DH
SCALE = 0.08838834764831843
LOG2E = 1.4426950408889634

BF16 = jnp.bfloat16
F32 = jnp.float32


def _rope_tables():
    inv = 1.0 / (10000.0 ** (np.arange(0, DH, 2) / DH))
    pos = np.arange(SQ)[:, None] * inv[None, :]
    cos = np.repeat(np.cos(pos), 2, axis=-1).astype(np.float32)
    sin = np.repeat(np.sin(pos), 2, axis=-1).astype(np.float32)
    sign = np.where(np.arange(DH) % 2 == 0, -1.0, 1.0).astype(np.float32)
    return np.stack([cos, sin * sign[None, :]]).astype(np.float32)


_TABLES = _rope_tables()


def pallas_dist_rope_attn_htp_bs_b2_sq512_d1024_hq8_dh128_kernel(
    x: jax.Array,
    Wq: jax.Array,
    Wk: jax.Array,
    Wv: jax.Array,
    Wo: jax.Array,
):
    def body(x_hbm, wq_hbm, wk_hbm, wv_hbm, wo_hbm, tab_ref, out_hbm,
             xs, wqkv, wo, wstage, xstage, tabs, q_s, k_s, v_s, ctx_s,
             res, snd, rcv, ostage,
             ld_sems, ag_send, ag_recv, rs_send, rs_recv, out_sems):
        me = lax.axis_index("i")
        left = lax.rem(me + N_DEV - 1, N_DEV)
        right = lax.rem(me + 1, N_DEV)

        def rdma(src, dst, ssem, rsem, dev):
            return pltpu.make_async_remote_copy(
                src_ref=src, dst_ref=dst, send_sem=ssem, recv_sem=rsem,
                device_id=(dev,), device_id_type=pl.DeviceIdType.MESH)

        ag = [
            rdma(xs.at[0], xs.at[2], ag_send.at[0], ag_recv.at[2], right),
            rdma(xs.at[7], xs.at[1], ag_send.at[1], ag_recv.at[1], left),
            rdma(xs.at[2], xs.at[3], ag_send.at[2], ag_recv.at[3], right),
            rdma(xs.at[1], xs.at[4], ag_send.at[3], ag_recv.at[4], left),
            rdma(xs.at[7], xs.at[6], ag_send.at[4], ag_recv.at[6], right),
            rdma(xs.at[0], xs.at[5], ag_send.at[5], ag_recv.at[5], left),
        ]
        ag_by_dst = {2: ag[0], 1: ag[1], 3: ag[2], 4: ag[3], 6: ag[4], 5: ag[5]}
        rs_plan = {1: (1, right), 2: (0, left), 3: (2, right), 4: (3, left),
                   5: (4, right), 6: (5, left)}
        rs = {u: rdma(snd.at[u], rcv.at[slot], rs_send.at[u], rs_recv.at[slot], dev)
              for u, (slot, dev) in rs_plan.items()}
        rs_by_slot = {slot: rs[u] for u, (slot, _) in rs_plan.items()}

        G = 2 * DH
        NG = HD // G
        ld_x = [pltpu.make_async_copy(x_hbm.at[b], xstage.at[b], ld_sems.at[b])
                for b in range(B_LOC)]
        ld_g = [[pltpu.make_async_copy(w.at[:, pl.ds(g * G, G)],
                                       wstage.at[j, :, pl.ds(g * G, G)],
                                       ld_sems.at[2 + 3 * g + j])
                 for j, w in enumerate((wq_hbm, wk_hbm, wv_hbm))]
                for g in range(NG)]
        ld_wo = pltpu.make_async_copy(wo_hbm, wstage.at[3], ld_sems.at[2 + 3 * NG])
        ld_x[0].start()
        for c in ld_g[0]:
            c.start()
        ld_x[1].start()

        barrier = pltpu.get_barrier_semaphore()
        for nbr in (left, right):
            pl.semaphore_signal(barrier, inc=1, device_id=(nbr,),
                                device_id_type=pl.DeviceIdType.MESH)

        tabs[0] = tab_ref[0]
        tabs[1] = tab_ref[1]
        tabs[2] = tab_ref[0] * (SCALE * LOG2E)
        tabs[3] = tab_ref[1] * (SCALE * LOG2E)
        rcv[6] = jnp.zeros((SQ, D), BF16)

        ld_x[0].wait()
        for c in ld_g[1]:
            c.start()
        xs[0] = xstage[0].astype(BF16)
        pl.semaphore_wait(barrier, 2)
        ag[0].start()

        def load_group(g):
            cols = slice(g * G, (g + 1) * G)
            for j in range(3):
                ld_g[g][j].wait()
                wqkv[j, :, cols] = wstage[j, :, cols].astype(BF16)
            if g == 0:
                ld_x[1].wait()
                xs[7] = xstage[1].astype(BF16)
                ag[1].start()
            if g + 2 < NG:
                for c in ld_g[g + 2]:
                    c.start()
            elif g + 2 == NG:
                ld_wo.start()

        def load_wo():
            ld_wo.wait()
            wo[...] = wstage[3].astype(BF16)

        even = (lax.broadcasted_iota(jnp.int32, (SQ, DH), 1) % 2) == 0

        def rope(t, c, s):
            sw = jnp.where(even, pltpu.roll(t, DH - 1, 1), pltpu.roll(t, 1, 1))
            return t * c + sw * s

        def compute(u, first=False):
            xu = xs[u]
            for g in range(NG):
                if first:
                    load_group(g)
                cols = slice(g * G, (g + 1) * G)
                q = jnp.dot(xu, wqkv[0, :, cols], preferred_element_type=F32)
                k = jnp.dot(xu, wqkv[1, :, cols], preferred_element_type=F32)
                v = jnp.dot(xu, wqkv[2, :, cols], preferred_element_type=F32)
                v_s[:, cols] = v.astype(BF16)
                for hh in range(2):
                    sl = slice(hh * DH, (hh + 1) * DH)
                    oc = slice(g * G + hh * DH, g * G + (hh + 1) * DH)
                    q_s[:, oc] = rope(q[:, sl], tabs[2], tabs[3]).astype(BF16)
                    k_s[:, oc] = rope(k[:, sl], tabs[0], tabs[1]).astype(BF16)
            if first:
                load_wo()
            for h in range(H_LOC):
                oc = slice(h * DH, (h + 1) * DH)
                s = lax.dot_general(q_s[:, oc], k_s[:, oc],
                                    (((1,), (1,)), ((), ())),
                                    preferred_element_type=F32)
                m = jnp.max(s, axis=-1, keepdims=True)
                p = jnp.exp2(s - m)
                l = jnp.sum(p, axis=-1, keepdims=True)
                o = jnp.dot(p.astype(BF16), v_s[:, oc], preferred_element_type=F32)
                ctx_s[:, oc] = (o / l).astype(BF16)
            KS = 6 * DH
            r = jnp.dot(ctx_s[:, :KS], wo[:KS, :], preferred_element_type=F32)
            return r + jnp.dot(ctx_s[:, KS:], wo[KS:, :], preferred_element_type=F32)

        res[0] = compute(0, first=True)
        ag_by_dst[2].wait_recv()
        ag[2].start()
        ag_by_dst[1].wait_recv()
        ag[3].start()
        ag[4].start()
        ag[5].start()

        def unit(u, carry):
            for k in (3, 4, 5, 6):
                @pl.when(u == k)
                def _():
                    ag_by_dst[k].wait_recv()
            for k, slot in ((5, 2), (6, 3), (7, 1)):
                @pl.when(u == k)
                def _():
                    rs_by_slot[slot].wait_recv()
            a = jnp.where(u == 5, 2, jnp.where(u == 6, 3, jnp.where(u == 7, 1, 6)))
            r = compute(u) + rcv[a].astype(F32)
            res[1] = r
            snd[u] = r.astype(BF16)
            for k in range(1, 7):
                @pl.when(u == k)
                def _():
                    rs[k].start()
            @pl.when(u == 6)
            def _():
                rs_by_slot[0].wait_recv()
                rs_by_slot[4].wait_recv()
                ostage[0] = res[0] + rcv[0].astype(F32) + rcv[4].astype(F32)
                pltpu.make_async_copy(ostage.at[0], out_hbm.at[0], out_sems.at[0]).start()
            return carry

        lax.fori_loop(1, 8, unit, 0)

        rs_by_slot[5].wait_recv()
        ostage[1] = res[1] + rcv[5].astype(F32)
        o1 = pltpu.make_async_copy(ostage.at[1], out_hbm.at[1], out_sems.at[1])
        o1.start()
        for c in ag:
            c.wait_send()
        for u in range(1, 7):
            rs[u].wait_send()
        pltpu.make_async_copy(ostage.at[0], out_hbm.at[0], out_sems.at[0]).wait()
        o1.wait()

    hbm = pl.BlockSpec(memory_space=pltpu.MemorySpace.HBM)
    return pl.pallas_call(
        body,
        out_shape=pltpu.HBM((B_LOC, SQ, D), F32),
        in_specs=[hbm, hbm, hbm, hbm, hbm,
                  pl.BlockSpec(memory_space=pltpu.VMEM)],
        out_specs=hbm,
        scratch_shapes=[
            pltpu.VMEM((8, SQ, D), BF16),
            pltpu.VMEM((3, D, HD), BF16),
            pltpu.VMEM((HD, D), BF16),
            pltpu.VMEM((4, D, HD), F32),
            pltpu.VMEM((2, SQ, D), F32),
            pltpu.VMEM((4, SQ, DH), F32),
            pltpu.VMEM((SQ, HD), BF16),
            pltpu.VMEM((SQ, HD), BF16),
            pltpu.VMEM((SQ, HD), BF16),
            pltpu.VMEM((SQ, HD), BF16),
            pltpu.VMEM((2, SQ, D), F32),
            pltpu.VMEM((8, SQ, D), BF16),
            pltpu.VMEM((7, SQ, D), BF16),
            pltpu.VMEM((2, SQ, D), F32),
            pltpu.SemaphoreType.DMA((15,)),
            pltpu.SemaphoreType.DMA((6,)),
            pltpu.SemaphoreType.DMA((8,)),
            pltpu.SemaphoreType.DMA((8,)),
            pltpu.SemaphoreType.DMA((6,)),
            pltpu.SemaphoreType.DMA((2,)),
        ],
        compiler_params=pltpu.CompilerParams(
            collective_id=0,
            vmem_limit_bytes=100 * 1024 * 1024,
        ),
    )(x, Wq, Wk, Wv, Wo, jnp.asarray(_TABLES))
```

```python
import numpy as np

import jax
import jax.numpy as jnp
from jax import lax
from jax.experimental import pallas as pl
from jax.experimental.pallas import tpu as pltpu

N_DEV = 4
B_LOC = 2
SQ = 512
D = 1024
H_LOC = 8
DH = 128
HD = H_LOC * DH
SCALE = 0.08838834764831843
LOG2E = 1.4426950408889634

BF16 = jnp.bfloat16
F32 = jnp.float32


def _rope_tables():
    inv = 1.0 / (10000.0 ** (np.arange(0, DH, 2) / DH))
    pos = np.arange(SQ)[:, None] * inv[None, :]
    cos = np.repeat(np.cos(pos), 2, axis=-1).astype(np.float32)
    sin = np.repeat(np.sin(pos), 2, axis=-1).astype(np.float32)
    sign = np.where(np.arange(DH) % 2 == 0, -1.0, 1.0).astype(np.float32)
    return np.stack([cos, sin * sign[None, :]]).astype(np.float32)


_TABLES = _rope_tables()


def pallas_dist_rope_attn_htp_bs_b2_sq512_d1024_hq8_dh128_kernel(
    x: jax.Array,
    Wq: jax.Array,
    Wk: jax.Array,
    Wv: jax.Array,
    Wo: jax.Array,
):
    def body(x_hbm, wq_hbm, wk_hbm, wv_hbm, wo_hbm, tab_ref, out_ref,
             xs, wqkv, wo, wstage, xstage, tabs, q_s, k_s, v_s, ctx_s,
             res, snd, rcv,
             ld_sems, ag_send, ag_recv, rs_send, rs_recv):
        me = lax.axis_index("i")
        left = lax.rem(me + N_DEV - 1, N_DEV)
        right = lax.rem(me + 1, N_DEV)

        def rdma(src, dst, ssem, rsem, dev):
            return pltpu.make_async_remote_copy(
                src_ref=src, dst_ref=dst, send_sem=ssem, recv_sem=rsem,
                device_id=(dev,), device_id_type=pl.DeviceIdType.MESH)

        ag = [
            rdma(xs.at[0], xs.at[4], ag_send.at[0], ag_recv.at[4], right),
            rdma(xs.at[7], xs.at[1], ag_send.at[1], ag_recv.at[1], left),
            rdma(xs.at[4], xs.at[2], ag_send.at[2], ag_recv.at[2], right),
            rdma(xs.at[1], xs.at[3], ag_send.at[3], ag_recv.at[3], left),
            rdma(xs.at[7], xs.at[6], ag_send.at[4], ag_recv.at[6], right),
            rdma(xs.at[0], xs.at[5], ag_send.at[5], ag_recv.at[5], left),
        ]
        ag_by_dst = {4: ag[0], 1: ag[1], 2: ag[2], 3: ag[3], 6: ag[4], 5: ag[5]}
        rs_plan = {1: (1, right), 4: (0, left), 2: (2, right), 3: (3, left),
                   5: (4, right), 6: (5, left)}
        rs = {u: rdma(snd.at[u], rcv.at[slot], rs_send.at[u], rs_recv.at[slot], dev)
              for u, (slot, dev) in rs_plan.items()}
        rs_by_slot = {slot: rs[u] for u, (slot, _) in rs_plan.items()}

        G = 2 * DH
        NG = HD // G
        ld_x = [pltpu.make_async_copy(x_hbm.at[b], xstage.at[b], ld_sems.at[b])
                for b in range(B_LOC)]
        ld_g = [[pltpu.make_async_copy(w.at[:, pl.ds(g * G, G)],
                                       wstage.at[j, :, pl.ds(g * G, G)],
                                       ld_sems.at[2 + 3 * g + j])
                 for j, w in enumerate((wq_hbm, wk_hbm, wv_hbm))]
                for g in range(NG)]
        ld_wo = pltpu.make_async_copy(wo_hbm, wstage.at[3], ld_sems.at[2 + 3 * NG])
        ld_x[0].start()
        for c in ld_g[0]:
            c.start()
        ld_x[1].start()

        barrier = pltpu.get_barrier_semaphore()
        for nbr in (left, right):
            pl.semaphore_signal(barrier, inc=1, device_id=(nbr,),
                                device_id_type=pl.DeviceIdType.MESH)

        tabs[0] = tab_ref[0]
        tabs[1] = tab_ref[1]
        tabs[2] = tab_ref[0] * (SCALE * LOG2E)
        tabs[3] = tab_ref[1] * (SCALE * LOG2E)
        rcv[6] = jnp.zeros((SQ, D), BF16)

        ld_x[0].wait()
        for c in ld_g[1]:
            c.start()
        xs[0] = xstage[0].astype(BF16)
        pl.semaphore_wait(barrier, 2)
        ag[0].start()

        def load_group(g):
            cols = slice(g * G, (g + 1) * G)
            for j in range(3):
                ld_g[g][j].wait()
                wqkv[j, :, cols] = wstage[j, :, cols].astype(BF16)
            if g == 0:
                ld_x[1].wait()
                xs[7] = xstage[1].astype(BF16)
                ag[1].start()
            if g + 2 < NG:
                for c in ld_g[g + 2]:
                    c.start()
            elif g + 2 == NG:
                ld_wo.start()

        def load_wo():
            ld_wo.wait()
            wo[...] = wstage[3].astype(BF16)

        even = (lax.broadcasted_iota(jnp.int32, (SQ, DH), 1) % 2) == 0

        def rope(t, c, s):
            sw = jnp.where(even, pltpu.roll(t, DH - 1, 1), pltpu.roll(t, 1, 1))
            return t * c + sw * s

        def compute(u, first=False):
            xu = xs[u]
            for g in range(NG):
              if first:
                  load_group(g)
              cols = slice(g * G, (g + 1) * G)
              q = jnp.dot(xu, wqkv[0, :, cols], preferred_element_type=F32)
              k = jnp.dot(xu, wqkv[1, :, cols], preferred_element_type=F32)
              v = jnp.dot(xu, wqkv[2, :, cols], preferred_element_type=F32)
              v_s[:, cols] = v.astype(BF16)
              for hh in range(2):
                  sl = slice(hh * DH, (hh + 1) * DH)
                  oc = slice(g * G + hh * DH, g * G + (hh + 1) * DH)
                  q_s[:, oc] = rope(q[:, sl], tabs[2], tabs[3]).astype(BF16)
                  k_s[:, oc] = rope(k[:, sl], tabs[0], tabs[1]).astype(BF16)
              for h in range(2 * g, 2 * g + 2):
                oc = slice(h * DH, (h + 1) * DH)
                s = lax.dot_general(q_s[:, oc], k_s[:, oc],
                                    (((1,), (1,)), ((), ())),
                                    preferred_element_type=F32)
                m = jnp.max(s, axis=-1, keepdims=True)
                p = jnp.exp2(s - m)
                l = jnp.sum(p, axis=-1, keepdims=True)
                o = jnp.dot(p.astype(BF16), v_s[:, oc], preferred_element_type=F32)
                ctx_s[:, oc] = (o / l).astype(BF16)
            if first:
                load_wo()
                ag_by_dst[4].wait_recv()
                ag[2].start()
                ag_by_dst[1].wait_recv()
                ag[3].start()
                ag[4].start()
                ag[5].start()
            KS = 6 * DH
            r = jnp.dot(ctx_s[:, :KS], wo[:KS, :], preferred_element_type=F32)
            return r + jnp.dot(ctx_s[:, KS:], wo[KS:, :], preferred_element_type=F32)

        res[0] = compute(0, first=True)

        def unit(u, carry):
            for k in (2, 3, 5, 6):
                @pl.when(u == k)
                def _():
                    ag_by_dst[k].wait_recv()
            for k, slot in ((5, 2), (6, 3), (7, 1)):
                @pl.when(u == k)
                def _():
                    rs_by_slot[slot].wait_recv()
            a = jnp.where(u == 5, 2, jnp.where(u == 6, 3, jnp.where(u == 7, 1, 6)))
            r = compute(u) + rcv[a].astype(F32)
            res[1] = r
            snd[u] = r.astype(BF16)
            for k in range(1, 7):
                @pl.when(u == k)
                def _():
                    rs[k].start()
            return carry

        lax.fori_loop(1, 8, unit, 0)

        rs_by_slot[0].wait_recv()
        rs_by_slot[4].wait_recv()
        out_ref[0] = res[0] + rcv[0].astype(F32) + rcv[4].astype(F32)
        rs_by_slot[5].wait_recv()
        out_ref[1] = res[1] + rcv[5].astype(F32)
        for c in ag:
            c.wait_send()
        for u in range(1, 7):
            rs[u].wait_send()

    hbm = pl.BlockSpec(memory_space=pltpu.MemorySpace.HBM)
    return pl.pallas_call(
        body,
        out_shape=jax.ShapeDtypeStruct((B_LOC, SQ, D), F32),
        in_specs=[hbm, hbm, hbm, hbm, hbm,
                  pl.BlockSpec(memory_space=pltpu.VMEM)],
        out_specs=pl.BlockSpec(memory_space=pltpu.VMEM),
        scratch_shapes=[
            pltpu.VMEM((8, SQ, D), BF16),
            pltpu.VMEM((3, D, HD), BF16),
            pltpu.VMEM((HD, D), BF16),
            pltpu.VMEM((4, D, HD), F32),
            pltpu.VMEM((2, SQ, D), F32),
            pltpu.VMEM((4, SQ, DH), F32),
            pltpu.VMEM((SQ, HD), BF16),
            pltpu.VMEM((SQ, HD), BF16),
            pltpu.VMEM((SQ, HD), BF16),
            pltpu.VMEM((SQ, HD), BF16),
            pltpu.VMEM((2, SQ, D), F32),
            pltpu.VMEM((8, SQ, D), BF16),
            pltpu.VMEM((7, SQ, D), BF16),
            pltpu.SemaphoreType.DMA((15,)),
            pltpu.SemaphoreType.DMA((6,)),
            pltpu.SemaphoreType.DMA((8,)),
            pltpu.SemaphoreType.DMA((8,)),
            pltpu.SemaphoreType.DMA((6,)),
        ],
        compiler_params=pltpu.CompilerParams(
            collective_id=0,
            vmem_limit_bytes=100 * 1024 * 1024,
        ),
    )(x, Wq, Wk, Wv, Wo, jnp.asarray(_TABLES))
```

```python
import numpy as np

import jax
import jax.numpy as jnp
from jax import lax
from jax.experimental import pallas as pl
from jax.experimental.pallas import tpu as pltpu

N_DEV = 4
B_LOC = 2
SQ = 512
D = 1024
H_LOC = 8
DH = 128
HD = H_LOC * DH
SCALE = 0.08838834764831843
LOG2E = 1.4426950408889634

BF16 = jnp.bfloat16
F32 = jnp.float32


def _rope_tables():
    inv = 1.0 / (10000.0 ** (np.arange(0, DH, 2) / DH))
    pos = np.arange(SQ)[:, None] * inv[None, :]
    cos = np.repeat(np.cos(pos), 2, axis=-1).astype(np.float32)
    sin = np.repeat(np.sin(pos), 2, axis=-1).astype(np.float32)
    sign = np.where(np.arange(DH) % 2 == 0, -1.0, 1.0).astype(np.float32)
    return np.stack([cos, sin * sign[None, :]]).astype(np.float32)


_TABLES = _rope_tables()


def pallas_dist_rope_attn_htp_bs_b2_sq512_d1024_hq8_dh128_kernel(
    x: jax.Array,
    Wq: jax.Array,
    Wk: jax.Array,
    Wv: jax.Array,
    Wo: jax.Array,
):
    def body(x_hbm, wq_hbm, wk_hbm, wv_hbm, wo_hbm, tab_ref, out_ref,
             xs, wqkv, wo, wstage, xstage, tabs, q_s, k_s, v_s, ctx_s,
             res, snd, rcv,
             ld_sems, ag_send, ag_recv, rs_send, rs_recv):
        me = lax.axis_index("i")
        left = lax.rem(me + N_DEV - 1, N_DEV)
        right = lax.rem(me + 1, N_DEV)

        def rdma(src, dst, ssem, rsem, dev):
            return pltpu.make_async_remote_copy(
                src_ref=src, dst_ref=dst, send_sem=ssem, recv_sem=rsem,
                device_id=(dev,), device_id_type=pl.DeviceIdType.MESH)

        ag = [
            rdma(xs.at[0], xs.at[1], ag_send.at[0], ag_recv.at[1], right),
            rdma(xs.at[7], xs.at[4], ag_send.at[1], ag_recv.at[4], left),
            rdma(xs.at[1], xs.at[2], ag_send.at[2], ag_recv.at[2], right),
            rdma(xs.at[4], xs.at[3], ag_send.at[3], ag_recv.at[3], left),
            rdma(xs.at[7], xs.at[6], ag_send.at[4], ag_recv.at[6], right),
            rdma(xs.at[0], xs.at[5], ag_send.at[5], ag_recv.at[5], left),
        ]
        ag_by_dst = {1: ag[0], 4: ag[1], 2: ag[2], 3: ag[3], 6: ag[4], 5: ag[5]}
        rs_plan = {4: (1, right), 1: (0, left), 2: (2, right), 3: (3, left),
                   5: (4, right), 6: (5, left)}
        rs = {u: rdma(snd.at[u], rcv.at[slot], rs_send.at[u], rs_recv.at[slot], dev)
              for u, (slot, dev) in rs_plan.items()}
        rs_by_slot = {slot: rs[u] for u, (slot, _) in rs_plan.items()}

        G = 2 * DH
        NG = HD // G
        ld_x = [pltpu.make_async_copy(x_hbm.at[b], xstage.at[b], ld_sems.at[b])
                for b in range(B_LOC)]
        ld_g = [[pltpu.make_async_copy(w.at[:, pl.ds(g * G, G)],
                                       wstage.at[j, :, pl.ds(g * G, G)],
                                       ld_sems.at[2 + 3 * g + j])
                 for j, w in enumerate((wq_hbm, wk_hbm, wv_hbm))]
                for g in range(NG)]
        ld_wo = pltpu.make_async_copy(wo_hbm, wstage.at[3], ld_sems.at[2 + 3 * NG])
        ld_x[0].start()
        for c in ld_g[0]:
            c.start()

        barrier = pltpu.get_barrier_semaphore()
        for nbr in (left, right):
            pl.semaphore_signal(barrier, inc=1, device_id=(nbr,),
                                device_id_type=pl.DeviceIdType.MESH)

        tabs[0] = tab_ref[0]
        tabs[1] = tab_ref[1]
        tabs[2] = tab_ref[0] * (SCALE * LOG2E)
        tabs[3] = tab_ref[1] * (SCALE * LOG2E)
        rcv[6] = jnp.zeros((SQ, D), BF16)

        ld_x[0].wait()
        xs[0] = xstage[0].astype(BF16)
        pl.semaphore_wait(barrier, 2)
        ag[0].start()

        def load_group(g):
            cols = slice(g * G, (g + 1) * G)
            for j in range(3):
                ld_g[g][j].wait()
                if j == 0:
                    if g + 1 < NG:
                        for c in ld_g[g + 1]:
                            c.start()
                    else:
                        ld_wo.start()
                wqkv[j, :, cols] = wstage[j, :, cols].astype(BF16)
            if g == 1:
                ld_x[1].start()
            if g == 2:
                ld_x[1].wait()
                xs[7] = xstage[1].astype(BF16)
                ag[1].start()

        def load_wo():
            ld_wo.wait()
            wo[...] = wstage[3].astype(BF16)

        even = (lax.broadcasted_iota(jnp.int32, (SQ, DH), 1) % 2) == 0

        def rope(t, c, s):
            sw = jnp.where(even, pltpu.roll(t, DH - 1, 1), pltpu.roll(t, 1, 1))
            return t * c + sw * s

        def proj(u, g, j):
            cols = slice(g * G, (g + 1) * G)
            t = jnp.dot(xs[u], wqkv[j, :, cols], preferred_element_type=F32)
            if j == 2:
                v_s[:, cols] = t.astype(BF16)
                return
            dst = (q_s, k_s)[j]
            for hh in range(2):
                sl = slice(hh * DH, (hh + 1) * DH)
                oc = slice(g * G + hh * DH, g * G + (hh + 1) * DH)
                dst[:, oc] = rope(t[:, sl], tabs[2 - 2 * j], tabs[3 - 2 * j]).astype(BF16)

        def scores(h):
            oc = slice(h * DH, (h + 1) * DH)
            s = lax.dot_general(q_s[:, oc], k_s[:, oc], (((1,), (1,)), ((), ())),
                                preferred_element_type=F32)
            m = jnp.max(s, axis=-1, keepdims=True)
            p = jnp.exp2(s - m)
            l = jnp.sum(p, axis=-1, keepdims=True)
            return p.astype(BF16), l

        def context(h, pl_):
            p, l = pl_
            oc = slice(h * DH, (h + 1) * DH)
            o = jnp.dot(p, v_s[:, oc], preferred_element_type=F32)
            ctx_s[:, oc] = (o / l).astype(BF16)

        def compute(u):
            for g in range(NG):
                for j in range(3):
                    if j == 0:
                        pl.when(u == 0)(lambda: load_group(g))
                    proj(u, g, j)
                if g > 0:
                    for h in (2 * g - 2, 2 * g - 1):
                        context(h, scores(h))

            @pl.when(u == 0)
            def _():
                load_wo()
                ag_by_dst[1].wait_recv()
                ag[2].start()
                ag[4].start()
                ag[5].start()

            for h in (H_LOC - 2, H_LOC - 1):
                context(h, scores(h))
            KS = 6 * DH
            r = jnp.dot(ctx_s[:, :KS], wo[:KS, :], preferred_element_type=F32)
            return r + jnp.dot(ctx_s[:, KS:], wo[KS:, :], preferred_element_type=F32)

        def unit(u, carry):
            for k in (2, 3, 5, 6):
                @pl.when(u == k)
                def _():
                    ag_by_dst[k].wait_recv()
            for k, slot in ((5, 2), (6, 3), (7, 1)):
                @pl.when(u == k)
                def _():
                    rs_by_slot[slot].wait_recv()
            a = jnp.where(u == 5, 2, jnp.where(u == 6, 3, jnp.where(u == 7, 1, 6)))
            r = compute(u) + rcv[a].astype(F32)
            res[jnp.minimum(u, 1)] = r
            snd[u] = r.astype(BF16)
            @pl.when(u == 1)
            def _():
                ag_by_dst[4].wait_recv()
                ag[3].start()
            for k in range(1, 7):
                @pl.when(u == k)
                def _():
                    rs[k].start()
            return carry

        lax.fori_loop(0, 8, unit, 0)

        rs_by_slot[0].wait_recv()
        rs_by_slot[4].wait_recv()
        out_ref[0] = res[0] + rcv[0].astype(F32) + rcv[4].astype(F32)
        rs_by_slot[5].wait_recv()
        out_ref[1] = res[1] + rcv[5].astype(F32)
        for c in ag:
            c.wait_send()
        for u in range(1, 7):
            rs[u].wait_send()

    hbm = pl.BlockSpec(memory_space=pltpu.MemorySpace.HBM)
    return pl.pallas_call(
        body,
        out_shape=jax.ShapeDtypeStruct((B_LOC, SQ, D), F32),
        in_specs=[hbm, hbm, hbm, hbm, hbm,
                  pl.BlockSpec(memory_space=pltpu.VMEM)],
        out_specs=pl.BlockSpec(memory_space=pltpu.VMEM),
        scratch_shapes=[
            pltpu.VMEM((8, SQ, D), BF16),
            pltpu.VMEM((3, D, HD), BF16),
            pltpu.VMEM((HD, D), BF16),
            pltpu.VMEM((4, D, HD), F32),
            pltpu.VMEM((2, SQ, D), F32),
            pltpu.VMEM((4, SQ, DH), F32),
            pltpu.VMEM((SQ, HD), BF16),
            pltpu.VMEM((SQ, HD), BF16),
            pltpu.VMEM((SQ, HD), BF16),
            pltpu.VMEM((SQ, HD), BF16),
            pltpu.VMEM((2, SQ, D), F32),
            pltpu.VMEM((8, SQ, D), BF16),
            pltpu.VMEM((7, SQ, D), BF16),
            pltpu.SemaphoreType.DMA((15,)),
            pltpu.SemaphoreType.DMA((6,)),
            pltpu.SemaphoreType.DMA((8,)),
            pltpu.SemaphoreType.DMA((8,)),
            pltpu.SemaphoreType.DMA((6,)),
        ],
        compiler_params=pltpu.CompilerParams(
            collective_id=0,
            vmem_limit_bytes=100 * 1024 * 1024,
        ),
    )(x, Wq, Wk, Wv, Wo, jnp.asarray(_TABLES))
```
